```python
import numpy as np

kernel_name = "dist_halo_stencil_i_m8192_n1024"

def setup_inputs():
    return {"x": np.random.randn(32768, 1024).astype(np.float32)}

def reference(x: np.ndarray) -> np.ndarray:
    out = np.empty_like(x)
    out[0] = x[0]
    out[-1] = x[-1]
    out[1:-1] = 0.25 * x[:-2] + 0.5 * x[1:-1] + 0.25 * x[2:]
    return out
```

```python
import jax
import jax.numpy as jnp
from jax import lax
from jax.experimental import pallas as pl
from jax.experimental.pallas import tpu as pltpu

N_DEV = 4
PAD = 8
GROUP = 128
BR = 16
ENDS = (2560, 3584, 3936, 4048, 4088)


def pallas_dist_halo_stencil_i_m8192_n1024_kernel(x: jax.Array):
    m, n = x.shape
    half = m // 2
    nch = len(ENDS)
    starts = (0,) + ENDS[:-1]

    def kernel_body(x_hbm, top, bot, xin, read_sem, send_sem, halo_sem):
        me = lax.axis_index("i")
        left, right = (me + N_DEV - 1) % N_DEV, (me + 1) % N_DEV

        def read(lo, hi, k):
            return pltpu.make_async_copy(
                x_hbm.at[pl.ds(lo, hi - lo)], xin.at[pl.ds(PAD + lo, hi - lo)], read_sem.at[k])

        read(half - 8, m, nch).start()
        for k in range(nch):
            read(starts[k], ENDS[k], k).start()

        bar = pltpu.get_barrier_semaphore()
        for nb in (left, right):
            pl.semaphore_signal(bar, 1, device_id=(nb,), device_id_type=pl.DeviceIdType.MESH)
        pl.semaphore_wait(bar, 2)
        up = pltpu.make_async_remote_copy(
            x_hbm.at[pl.ds(0, 1)], xin.at[pl.ds(PAD + m, 1)], send_sem.at[0], halo_sem.at[0],
            device_id=(left,), device_id_type=pl.DeviceIdType.MESH)
        down = pltpu.make_async_remote_copy(
            x_hbm.at[pl.ds(m - 1, 1)], xin.at[pl.ds(PAD - 1, 1)], send_sem.at[1], halo_sem.at[1],
            device_id=(right,), device_id_type=pl.DeviceIdType.MESH)
        up.start()
        down.start()
        up.wait()
        down.wait()

        def block(out, r, base):
            r = pl.multiple_of(r, BR)
            w = xin[pl.ds(base + r, BR + 16), :]
            q = 0.25 * w
            y = (q[7:7 + BR] + 0.5 * w[8:8 + BR]) + q[9:9 + BR]
            out[r // GROUP, pl.ds(pl.multiple_of(r % GROUP, BR), BR), :] = y

        read(half - 8, m, nch).wait()
        lax.fori_loop(0, half // BR, lambda i, _: block(bot, i * BR, half), None)

        @pl.when(me == N_DEV - 1)
        def _():
            bot[half // GROUP - 1, GROUP - 1:GROUP, :] = xin[PAD + m - 1:PAD + m, :]

        done = 0
        for k in range(nch):
            read(starts[k], ENDS[k], k).wait()
            upto = half // BR if k == nch - 1 else (ENDS[k] - 8) // BR
            lax.fori_loop(done, upto, lambda i, _: block(top, i * BR, 0), None)
            done = upto
            if k == 0:
                @pl.when(me == 0)
                def _():
                    top[0, 0:1, :] = xin[PAD:PAD + 1, :]

    out = pltpu.VMEM((half // GROUP, GROUP, n), x.dtype)
    top, bot = pl.pallas_call(
        kernel_body,
        out_shape=[out, out],
        in_specs=[pl.BlockSpec(memory_space=pl.ANY)],
        out_specs=[pl.BlockSpec(memory_space=pltpu.VMEM)] * 2,
        scratch_shapes=[
            pltpu.VMEM((m + 2 * PAD, n), x.dtype),
            pltpu.SemaphoreType.DMA((nch + 1,)),
            pltpu.SemaphoreType.DMA((2,)),
            pltpu.SemaphoreType.DMA((2,)),
        ],
        compiler_params=pltpu.CompilerParams(
            vmem_limit_bytes=40 * 2**20, collective_id=0, disable_bounds_checks=True),
    )(x)
    return jnp.concatenate([top, bot], axis=0).reshape(m, n)
```

```python
import jax
import jax.numpy as jnp
from jax import lax
from jax.experimental import pallas as pl
from jax.experimental.pallas import tpu as pltpu

N_DEV = 4
SUB, LANE = 8, 128
GROUP_ROWS = 256
COL_BLOCKS = 4
STEP_ROWS = 32
READ_ENDS = (2152, 3368, 3848, 4008, 4040, 4072, 4088)


def pallas_dist_halo_stencil_i_m8192_n1024_kernel(x: jax.Array):
    m, n = x.shape
    half = m // 2
    width = n // COL_BLOCKS
    assert READ_ENDS[-1] == half - SUB
    reads = [(READ_ENDS[-1], m)] + list(zip((0,) + READ_ENDS[:-1], READ_ENDS))

    def kernel_body(x_hbm, *refs):
        upper, lower = refs[:COL_BLOCKS], refs[COL_BLOCKS : 2 * COL_BLOCKS]
        x_vmem, read_sems, send_sems, recv_sems = refs[2 * COL_BLOCKS :]

        copies = [
            pltpu.make_async_copy(
                x_hbm.at[pl.ds(lo, hi - lo)],
                x_vmem.at[pl.ds(SUB + lo, hi - lo)],
                read_sems.at[k],
            )
            for k, (lo, hi) in enumerate(reads)
        ]
        for copy in copies:
            copy.start()

        x_vmem[:SUB, :] = jnp.zeros((SUB, n), x.dtype)
        x_vmem[SUB + m :, :] = jnp.zeros((SUB, n), x.dtype)

        me = lax.axis_index("i")
        prev_dev, next_dev = (me + N_DEV - 1) % N_DEV, (me + 1) % N_DEV
        barrier = pltpu.get_barrier_semaphore()
        for dev in (prev_dev, next_dev):
            pl.semaphore_signal(
                barrier, 1, device_id=(dev,), device_id_type=pl.DeviceIdType.MESH
            )
        pl.semaphore_wait(barrier, 2)

        halos = [
            pltpu.make_async_remote_copy(
                x_hbm.at[pl.ds(src_row, 1)],
                x_vmem.at[pl.ds(dst_row, 1)],
                send_sems.at[k],
                recv_sems.at[k],
                device_id=(dev,),
                device_id_type=pl.DeviceIdType.MESH,
            )
            for k, (src_row, dst_row, dev) in enumerate(
                [(0, SUB + m, prev_dev), (m - 1, SUB - 1, next_dev)]
            )
        ]
        for halo in halos:
            halo.start()
        for halo in halos:
            halo.wait()

        sublane = lax.broadcasted_iota(jnp.int32, (SUB, LANE), 0)

        def stencil(out, first_row, lo, hi):
            def step(i, _):
                row = pl.multiple_of(i * STEP_ROWS, STEP_ROWS)
                group = row // GROUP_ROWS
                offset = pl.multiple_of(row % GROUP_ROWS, STEP_ROWS)
                tiles = STEP_ROWS // SUB
                for col in range(0, n, LANE):
                    v = [
                        x_vmem[pl.ds(first_row + row + SUB * t, SUB), col : col + LANE]
                        for t in range(tiles + 2)
                    ]
                    q = [0.25 * u for u in v]
                    for t in range(1, tiles + 1):
                        above = jnp.where(sublane == SUB - 1, q[t - 1], q[t])
                        below = jnp.where(sublane == 0, q[t + 1], q[t])
                        out[col // width][
                            group,
                            pl.ds(offset + SUB * (t - 1), SUB),
                            pl.ds(col % width, LANE),
                        ] = (pltpu.roll(above, 1, 0) + 0.5 * v[t]) + pltpu.roll(
                            below, SUB - 1, 0
                        )

            lax.fori_loop(lo // STEP_ROWS, hi // STEP_ROWS, step, None)

        def keep_row(out, first_row, row):
            src = SUB + first_row + row
            for j in range(COL_BLOCKS):
                out[j][row // GROUP_ROWS, pl.ds(row % GROUP_ROWS, 1), :] = x_vmem[
                    pl.ds(src, 1), pl.ds(j * width, width)
                ]

        copies[0].wait()
        stencil(lower, half, 0, half)
        pl.when(me == N_DEV - 1)(lambda: keep_row(lower, half, half - 1))

        done = 0
        for copy, end in zip(copies[1:], READ_ENDS):
            ready = half if end == READ_ENDS[-1] else end - SUB
            copy.wait()
            stencil(upper, 0, done, ready)
            if done == 0:
                pl.when(me == 0)(lambda: keep_row(upper, 0, 0))
            done = ready

    block = pltpu.VMEM((half // GROUP_ROWS, GROUP_ROWS, width), x.dtype)
    blocks = pl.pallas_call(
        kernel_body,
        out_shape=[block] * (2 * COL_BLOCKS),
        in_specs=[pl.BlockSpec(memory_space=pl.ANY)],
        out_specs=[pl.BlockSpec(memory_space=pltpu.VMEM)] * (2 * COL_BLOCKS),
        scratch_shapes=[
            pltpu.VMEM((m + 2 * SUB, n), x.dtype),
            pltpu.SemaphoreType.DMA((len(reads),)),
            pltpu.SemaphoreType.DMA((2,)),
            pltpu.SemaphoreType.DMA((2,)),
        ],
        compiler_params=pltpu.CompilerParams(
            vmem_limit_bytes=40 * 2**20,
            collective_id=0,
            disable_bounds_checks=True,
            disable_semaphore_checks=True,
        ),
    )(x)
    halves = [
        jnp.concatenate(blocks[:COL_BLOCKS], axis=2),
        jnp.concatenate(blocks[COL_BLOCKS:], axis=2),
    ]
    return jnp.concatenate(halves, axis=0).reshape(m, n)
```

```python
import jax
import jax.numpy as jnp
from jax import lax
from jax.experimental import pallas as pl
from jax.experimental.pallas import tpu as pltpu

N_DEV = 4
SUB, LANE = 8, 128
GROUP_ROWS = 256
COL_BLOCKS = 4
STEP_ROWS = 32
READ_ENDS = (2152, 3336, 3816, 4008, 4072, 4088)
READS_IN_FLIGHT = 3


def pallas_dist_halo_stencil_i_m8192_n1024_kernel(x: jax.Array):
    m, n = x.shape
    half = m // 2
    width = n // COL_BLOCKS
    assert READ_ENDS[-1] == half - SUB
    reads = [(READ_ENDS[-1], m)] + list(zip((0,) + READ_ENDS[:-1], READ_ENDS))

    def kernel_body(x_hbm, *refs):
        upper, lower = refs[:COL_BLOCKS], refs[COL_BLOCKS : 2 * COL_BLOCKS]
        x_vmem, read_sems = refs[2 * COL_BLOCKS :]

        copies = [
            pltpu.make_async_copy(
                x_hbm.at[pl.ds(lo, hi - lo)],
                x_vmem.at[pl.ds(SUB + lo, hi - lo)],
                read_sems.at[k % READS_IN_FLIGHT],
            )
            for k, (lo, hi) in enumerate(reads)
        ]
        for copy in copies[:READS_IN_FLIGHT]:
            copy.start()

        def wait_read(k):
            copies[k].wait()
            if k + READS_IN_FLIGHT < len(copies):
                copies[k + READS_IN_FLIGHT].start()

        x_vmem[:SUB, :] = jnp.zeros((SUB, n), x.dtype)
        x_vmem[SUB + m :, :] = jnp.zeros((SUB, n), x.dtype)

        me = lax.axis_index("i")
        prev_dev, next_dev = (me + N_DEV - 1) % N_DEV, (me + 1) % N_DEV

        def exchange_halos(send_sems, recv_sems):
            barrier = pltpu.get_barrier_semaphore()
            for dev in (prev_dev, next_dev):
                pl.semaphore_signal(
                    barrier, 1, device_id=(dev,), device_id_type=pl.DeviceIdType.MESH
                )
            pl.semaphore_wait(barrier, 2)

            halos = [
                pltpu.make_async_remote_copy(
                    x_hbm.at[pl.ds(src_row, 1)],
                    x_vmem.at[pl.ds(dst_row, 1)],
                    send_sems.at[k],
                    recv_sems.at[k],
                    device_id=(dev,),
                    device_id_type=pl.DeviceIdType.MESH,
                )
                for k, (src_row, dst_row, dev) in enumerate(
                    [(0, SUB + m, prev_dev), (m - 1, SUB - 1, next_dev)]
                )
            ]
            for halo in halos:
                halo.start()
            for halo in halos:
                halo.wait()

        pl.run_scoped(
            exchange_halos, pltpu.SemaphoreType.DMA((2,)), pltpu.SemaphoreType.DMA((2,))
        )

        sublane = lax.broadcasted_iota(jnp.int32, (SUB, LANE), 0)

        def stencil(out, first_row, lo, hi):
            def step(i, _):
                row = pl.multiple_of(i * STEP_ROWS, STEP_ROWS)
                group = row // GROUP_ROWS
                offset = pl.multiple_of(row % GROUP_ROWS, STEP_ROWS)
                tiles = STEP_ROWS // SUB
                for col in range(0, n, LANE):
                    v = [
                        x_vmem[pl.ds(first_row + row + SUB * t, SUB), col : col + LANE]
                        for t in range(tiles + 2)
                    ]
                    q = [0.25 * u for u in v]
                    for t in range(1, tiles + 1):
                        above = jnp.where(sublane == SUB - 1, q[t - 1], q[t])
                        below = jnp.where(sublane == 0, q[t + 1], q[t])
                        out[col // width][
                            group,
                            pl.ds(offset + SUB * (t - 1), SUB),
                            pl.ds(col % width, LANE),
                        ] = (pltpu.roll(above, 1, 0) + 0.5 * v[t]) + pltpu.roll(
                            below, SUB - 1, 0
                        )

            lax.fori_loop(lo // STEP_ROWS, hi // STEP_ROWS, step, None)

        def keep_row(out, first_row, row):
            src = SUB + first_row + row
            for j in range(COL_BLOCKS):
                out[j][row // GROUP_ROWS, pl.ds(row % GROUP_ROWS, 1), :] = x_vmem[
                    pl.ds(src, 1), pl.ds(j * width, width)
                ]

        wait_read(0)
        stencil(lower, half, 0, half)
        pl.when(me == N_DEV - 1)(lambda: keep_row(lower, half, half - 1))

        done = 0
        for k, end in enumerate(READ_ENDS, start=1):
            ready = half if end == READ_ENDS[-1] else end - SUB
            wait_read(k)
            stencil(upper, 0, done, ready)
            if done == 0:
                pl.when(me == 0)(lambda: keep_row(upper, 0, 0))
            done = ready

    block = jax.ShapeDtypeStruct((half // GROUP_ROWS, GROUP_ROWS, width), x.dtype)
    blocks = pl.pallas_call(
        kernel_body,
        out_shape=[block] * (2 * COL_BLOCKS),
        in_specs=[pl.BlockSpec(memory_space=pl.ANY)],
        out_specs=[pl.BlockSpec(memory_space=pltpu.VMEM)] * (2 * COL_BLOCKS),
        scratch_shapes=[
            pltpu.VMEM((m + 2 * SUB, n), x.dtype),
            pltpu.SemaphoreType.DMA((READS_IN_FLIGHT,)),
        ],
        compiler_params=pltpu.CompilerParams(
            vmem_limit_bytes=40 * 2**20,
            collective_id=0,
        ),
    )(x)
    halves = [
        jnp.concatenate(blocks[:COL_BLOCKS], axis=2),
        jnp.concatenate(blocks[COL_BLOCKS:], axis=2),
    ]
    return jnp.concatenate(halves, axis=0).reshape(m, n)
```
